```python
import numpy as np

kernel_name = "dist_moe_cap_ep_tokshard_n2048_d512_e8_h1024"

def setup_inputs():
    x = np.random.randn(8192, 512).astype(np.float32)
    router_W = np.random.randn(512, 32).astype(np.float32) * 0.1
    scores64 = x.astype(np.float64) @ router_W.astype(np.float64)
    route_idx = np.argsort(-scores64, axis=-1)[:, :1].astype(np.int32)
    expert_W = np.random.randn(32, 512, 1024).astype(np.float32) * 0.02
    return {"x": x, "router_W": router_W, "route_idx": route_idx, "expert_W": expert_W}

def reference(x, router_W, route_idx, expert_W):
    counts = np.zeros(32, dtype=np.int64)
    out = np.zeros((8192, 1024), dtype=np.float32)
    for i in range(8192):
        e = int(route_idx[i, 0])
        if counts[e] < 204:
            out[i] = x[i] @ expert_W[e]
            counts[e] += 1
    return out
```

```python
import jax
import jax.numpy as jnp
from jax import lax
from jax.experimental import pallas as pl
from jax.experimental.pallas import tpu as pltpu

NDEV = 4
NT = 2048
DM = 512
DH = 1024
NE = 8
CAP = 204
CP = 208
XR = DM // 256
YR = DH // 256

CD = 16
CR = 32
GD = 4
GR = 2
DCOPY = 16
RCOPY = 8
NROW = NT // 128

PACE_D = {(2, 3): (2, 4), (2, 1): (6, 4)}
PACE_D_DEFAULT = (14, 2)
PACE_F = {0: (14, 2), 1: (6, 4), 2: (4, 2), 3: (0, 3)}
PACE_G = {0: (0, 1), 1: (-2, 0), 2: (-2, 0), 3: (-2, 0)}
MAX_BY_Y = 31
FIRST_RESULT = 390
LAG = {0: (0, 0, 8, 1), 1: (0, 0, 3, 1), 2: (0, 1, 8, 1), 3: (0, 1, 8, 1)}

TRAILING, BEFORE_END = 1, 2
LEAD_E, LEAD_ROWS, EARLY_PACK = 2, 9, 8
CHECKS = False

MESH = pl.DeviceIdType.MESH

MAXS = NE * CAP
NCD = -(-MAXS // CD)
NCR = -(-MAXS // CR)
LD = NCD * CD + CD
LR = NCR * CR + CR
D_FIRST = CD
D_DUMMY = D_FIRST + 8 * LD
assert MAXS <= 16 * 128 and DCOPY <= CD
DISPATCH, RETURN = (CD, GD), (CR, GR)


def _pick(idx, values):
  out = jnp.asarray(values[-1], jnp.int32)
  for i in range(len(values) - 2, -1, -1):
    out = jnp.where(idx == i, jnp.asarray(values[i], jnp.int32), out)
  return out


def _per_chip(me, fn):
  return _pick(me, [fn(m) for m in range(NDEV)])


def _cdiv_pow2(a, b):
  return (a + (b - 1)) >> (b.bit_length() - 1)


def _pack(lo, hi):
  bits = lambda v: lax.bitcast_convert_type(
      v.astype(jnp.bfloat16).astype(jnp.float32), jnp.int32)
  return lax.shift_right_logical(bits(lo), 16) | (bits(hi) & -65536)


def _unpack(words, index):
  bits = words & -65536 if index else words << 16
  return lax.bitcast_convert_type(bits, jnp.float32)


def _loop(lo, hi, body):
  def step(i, carry):
    body(i)
    return carry

  lax.fori_loop(lo, hi, step, 0)


def _short(left, kind, fn):
  chunk, gran = kind
  for size in range(gran, chunk, gran):
    pl.when((left > size - gran) & (left <= size))(lambda size=size: fn(size))


def _sized(left, kind, fn):
  chunk, gran = kind
  pl.when(left > chunk - gran)(lambda: fn(chunk))
  pl.when(left <= chunk - gran)(lambda: _short(left, kind, fn))


def _moe_kernel(
    x_hbm, route_hbm, w_hbm, out,
    xbuf, wbuf, route_v, xs, dbuf, rbuf, xe, ybuf,
    cnt_v, row_v, posd_v, meta_v, home_v,
    posd_s, meta_s, home_s,
    x_sem, w_sem, loc_sem, cnt_sem, small_send,
    d_send, r_send, d_recv, d_pass, r_recv, r_pass,
):
  me = lax.axis_index("i")

  def remote(src, dst, send_sem, recv_sem, rel):
    return pltpu.make_async_remote_copy(
        src, dst, send_sem, recv_sem, device_id=(me ^ rel,), device_id_type=MESH
    )

  route_cp = pltpu.make_async_copy(route_hbm, route_v, loc_sem.at[0])
  route_cp.start()

  def x_copy(b):
    rows = pl.ds(b * 128, 128)
    return pltpu.make_async_copy(x_hbm.at[rows], xbuf.at[rows], x_sem.at[b])

  def w_copy(j):
    return pltpu.make_async_copy(w_hbm.at[j], wbuf.at[j], w_sem.at[j])

  for b in range(NROW):
    x_copy(b).start(priority=1)
  barrier = pltpu.get_barrier_semaphore()
  for rel in (2, 3, 1):
    pl.semaphore_signal(barrier, 1, device_id=(me ^ rel,), device_id_type=MESH)
  route_cp.wait()

  expert = route_v[...] & (NDEV * NE - 1)
  sub32 = lax.broadcasted_iota(jnp.int32, (32, 128), 0)
  lane32 = lax.broadcasted_iota(jnp.int32, (32, 128), 1)
  tri_r = lax.broadcasted_iota(jnp.int32, (128, 256), 0)
  tri_c = lax.broadcasted_iota(jnp.int32, (128, 256), 1)
  prefix_total = jnp.where((tri_r < tri_c), 1.0, 0.0).astype(jnp.bfloat16)

  def prefix_counts(masks):
    onehot = jnp.concatenate([jnp.where(m, 1.0, 0.0) for m in masks], axis=0)
    return jnp.dot(
        onehot.astype(jnp.bfloat16), prefix_total,
        preferred_element_type=jnp.float32,
    )

  def pick_rows(mask, values):
    return jnp.sum(jnp.where(mask, values, 0.0), axis=0, keepdims=True)

  hot = [expert[r:r + 1, :] == sub32 for r in range(NROW)]
  sums = prefix_counts(hot)
  seen = jnp.zeros((32, 128), jnp.float32)
  for r in range(NROW):
    part = sums[32 * r:32 * (r + 1)]
    row_v[0, r:r + 1, :] = pick_rows(hot[r], part[:, :128] + seen)
    seen = seen + part[:, 128:]
    if r == LEAD_ROWS - 1:
      seen_lead = seen
  byte = lambda v: jnp.minimum(v, 255.0).astype(jnp.int32)
  counts = byte(seen) + (byte(seen_lead) << 8)
  cnt_v[0] = counts[:16] + (counts[16:] << 16)

  def cnt_copy(rel):
    return remote(cnt_v.at[0], cnt_v.at[rel], small_send, cnt_sem.at[rel], rel)

  pl.semaphore_wait(barrier, NDEV - 1)
  for rel in (2, 3, 1):
    cnt_copy(rel).start()

  def pack_block(b):
    t = b * 128
    for h in range(XR):
      lo = xbuf[t:t + 128, 256 * h:256 * h + 128]
      hi = xbuf[t:t + 128, 256 * h + 128:256 * h + 256]
      xs[pl.ds(t * XR + h, 128, stride=XR), :] = _pack(lo, hi)

  for b in range(EARLY_PACK):
    x_copy(b).wait()
    pack_block(b)
  for rel in (1, 2, 3):
    cnt_copy(rel).wait_recv()

  def running(v):
    for shift in (1, 2, 4):
      v = v + jnp.where((sub32 & 7) >= shift, pltpu.roll(v, shift, 0), 0)
    return v

  before = jnp.zeros((32, 128), jnp.int32)
  meta = my_keep = my_lead = before
  for s in range(NDEV):
    words = cnt_v[s ^ me]
    counts = jnp.concatenate([words, words >> 16], axis=0)
    keep = jnp.clip(CAP - before, 0, counts & 255)
    lead = jnp.minimum(keep, (counts >> 8) & 255)
    meta = jnp.where(
        lane32 == s, keep, jnp.where(lane32 == NDEV + s, lead, meta))
    my_keep = jnp.where(me == s, keep, my_keep)
    my_lead = jnp.where(me == s, lead, my_lead)
    before = before + (counts & 255)
  meta_v[...] = running(meta)

  my_start = running(my_keep) - my_keep
  lead_end = running(my_lead)
  leads = (sub32 & 7) < LEAD_E
  all_leads = jnp.where(leads, my_lead, 0)
  for shift in (1, 2, 4):
    all_leads = all_leads + jnp.where(
        (sub32 & shift) == 0, pltpu.roll(all_leads, 32 - shift, 0),
        pltpu.roll(all_leads, shift, 0))
  starts = (jnp.where(leads, lead_end - my_lead, my_start),
            jnp.where(leads, all_leads + my_start - lead_end, my_start))
  starts = [(v * 256 + my_keep).astype(jnp.float32) for v in starts]
  for r in range(NROW):
    row_v[1, r:r + 1, :] = pick_rows(hot[r], starts[int(r >= LEAD_ROWS)])
  rank = row_v[0].astype(jnp.int32)
  looked = row_v[1].astype(jnp.int32)
  kept = rank < (looked & 255)
  owner_rel = (expert >> 3) ^ me
  d_slot = jnp.where(owner_rel == 0, 0, owner_rel + 3)
  posd_v[...] = jnp.where(
      kept, D_FIRST + d_slot * LD + (looked >> 8) + rank, D_DUMMY) * XR
  posd_cp = pltpu.make_async_copy(posd_v, posd_s, loc_sem.at[1])
  posd_cp.start()
  ends_cp = pltpu.make_async_copy(meta_v, meta_s, loc_sem.at[2])
  ends_cp.start()
  posd_cp.wait()

  def sort_blocks(lo, hi):
    for b in range(lo, hi):
      if b >= EARLY_PACK:
        x_copy(b).wait()
        pack_block(b)
      if b == NROW - 1:
        for j in range(NE):
          w_copy(j).start()
      for l in range(128):
        t = b * 128 + l
        dbuf[pl.ds(posd_s[b, l], XR), :] = xs[t * XR:(t + 1) * XR, :]

  sort_blocks(0, LEAD_ROWS)
  ends_cp.wait()

  def end_of(s, d, j):
    return meta_s[d * NE + j, s]

  def total(s, d):
    return end_of(s, d, NE - 1)

  def lead_end_of(s, d, j):
    return meta_s[d * NE + j, NDEV + s]

  def d_chunks(s, d, j):
    upto = jnp.clip(j, 0, NE - 1)
    later_leads = (lead_end_of(s, d, LEAD_E - 1)
                   - lead_end_of(s, d, jnp.minimum(upto, LEAD_E - 1)))
    n = _cdiv_pow2(end_of(s, d, upto) + later_leads, CD)
    return jnp.where(j < 0, 0, n)

  def pace(table):
    a = _per_chip(me, lambda m: table(m)[0])
    b = _per_chip(me, lambda m: table(m)[1])
    return lambda j: jnp.where(j < 0, -1, (a + b * j) >> 1)

  def d_pace(src_rel, dst_rel):
    wanted = pace(
        lambda m: PACE_D.get((m ^ src_rel, m ^ dst_rel), PACE_D_DEFAULT))
    return lambda j: jnp.maximum(wanted(j), j)

  own_pace = {rel: d_pace(0, rel) for rel in (1, 2, 3)}
  passing_pace = d_pace(3, 1)
  forward_pace = pace(lambda m: PACE_F[m])
  result_pace = pace(lambda m: PACE_G[m])

  def d_sent(rel, j):
    return d_chunks(me, me ^ rel, own_pace[rel](j))

  def d_forwarded(j):
    upto = jnp.maximum(forward_pace(j), j)
    return d_chunks(me ^ 3, me ^ 1, jnp.minimum(upto, passing_pace(j)))

  def r_chunks(s, d, j):
    whole = end_of(s, d, jnp.clip(j, 0, NE - 1)) >> (CR.bit_length() - 1)
    return jnp.where(j >= NE - 1, _cdiv_pow2(total(s, d), CR),
                     jnp.where(j < 0, 0, whole))

  def r_forwarded(j):
    return r_chunks(me ^ 1, me ^ 3, jnp.minimum(result_pace(j), j))

  def plan_detours():
    load = {}
    for a in range(NDEV):
      for b, first in ((a ^ 3, a), (a ^ 1, a ^ 3)):
        out_kib = total(a, b) + total(first, first ^ 2)
        back_kib = 2 * (total(b, a) + total(first ^ 2, first))
        load[a, b] = jnp.maximum(out_kib, FIRST_RESULT) + back_kib
    tries = (sub32, lane32 & MAX_BY_Y)
    split = [None] * NDEV
    for pair in ((2, 3), (0, 1)):
      def moved(link, counts):
        kib = load[link]
        for d, count in zip(pair, counts):
          if link in ((d, d ^ 3), (d ^ 3, d ^ 2)):
            kib = kib - count * (2 * CR)
          elif link in ((d, d ^ 1), (d ^ 1, d ^ 2)):
            kib = kib + count * (2 * CR)
        return kib

      busiest = jnp.zeros((32, 128), jnp.int32)
      for a, b in load:
        if a in pair or a ^ b == 1:
          busiest = jnp.maximum(busiest, moved((a, b), tries))
      score = busiest + tries[0] + tries[1]
      score = (score << 10) + (tries[0] << 5) + tries[1]
      chunks = [_cdiv_pow2(total(d ^ 2, d), CR) for d in pair]
      possible = (tries[0] <= chunks[0]) & (tries[1] <= chunks[1])
      score = jnp.where(possible, score, (1 << 24) - 1).astype(jnp.float32)
      best = jnp.min(score).astype(jnp.int32)
      counts = ((best >> 5) & MAX_BY_Y, best & MAX_BY_Y)
      load = {link: moved(link, counts) for link in load}
      for d, n, count in zip(pair, chunks, counts):
        split[d] = n - count
    return split

  def d_rows(slot, c, size):
    start = pl.multiple_of((D_FIRST + slot * LD + c * CD) * XR, CD * XR)
    return dbuf.at[pl.ds(start, size * XR)]

  def r_rows(slot, c, size):
    start = pl.multiple_of((slot * LR + c * CR) * YR, CR * YR)
    return rbuf.at[pl.ds(start, size * YR)]

  def d_sem0(rel, d):
    return sum(_cdiv_pow2(total(d ^ k, d), CD) for k in range(1, rel))

  def r_sem0(rel, s):
    return sum(_cdiv_pow2(total(s, s ^ k), CR) for k in range(1, rel))

  d_out = {rel: d_sem0(rel, me ^ rel) for rel in (1, 3)}
  d_on = d_sem0(2, me ^ 1)
  d_in = {rel: d_sem0(rel, me) for rel in (1, 2, 3)}
  r_out = {rel: r_sem0(rel, me ^ rel) for rel in (1, 3)}
  r_on = {rel: r_sem0(2, me ^ rel ^ 2) for rel in (1, 3)}
  r_in = [0] + [r_sem0(rel, me) for rel in (1, 2, 3)]

  def d_own(rel, c, size):
    if rel == 2:
      return remote(d_rows(5, c, size), d_rows(7, c, size), d_send,
                    d_pass.at[c], 3)
    return remote(d_rows(3 + rel, c, size), d_rows(rel, c, size), d_send,
                  d_recv.at[d_out[rel] + c], rel)

  def d_fwd(c, size):
    return remote(d_rows(7, c, size), d_rows(2, c, size), d_send,
                  d_recv.at[d_on + c], 1)

  def r_own(rel, c, size):
    return remote(r_rows(3 + rel, c, size), r_rows(rel, c, size), r_send,
                  r_recv.at[r_out[rel] + c], rel)

  def r_diag(via, c, size, sender):
    sem = NCR + c - split[sender] if via == 1 else c
    return remote(r_rows(5, c, size), r_rows(7 + via // 2, c, size), r_send,
                  r_pass.at[sem], via)

  def r_fwd(src_rel, c, size):
    k = src_rel // 2
    return remote(r_rows(7 + k, c, size), r_rows(2, c, size), r_send,
                  r_recv.at[r_on[src_rel] + c], src_rel ^ 2)

  def interleaved(ranges, kind):
    chunk, gran = kind
    whole = [jnp.minimum(hi, (tokens + gran - 1) >> (chunk.bit_length() - 1))
             for _, hi, tokens, _ in ranges]
    if len(ranges) == 1:
      _loop(ranges[0][0], whole[0], lambda c: ranges[0][3](c, chunk))
    else:
      def turn(k):
        for (lo, _, _, fn), end in zip(ranges, whole):
          pl.when(lo + k < end)(lambda lo=lo, fn=fn: fn(lo + k, chunk))

      longest = jnp.int32(0)
      for (lo, _, _, _), end in zip(ranges, whole):
        longest = jnp.maximum(longest, end - lo)
      _loop(0, longest, turn)
    for (lo, hi, tokens, fn), end in zip(ranges, whole):
      pl.when((lo <= end) & (end < hi))(
          lambda end=end, tokens=tokens, fn=fn: _short(
              tokens - end * chunk, kind, lambda size: fn(end, size)))

  def each_chunk(lo, hi, tokens, kind, fn):
    interleaved([(lo, hi, tokens, fn)], kind)

  sent_early = {
      rel: lead_end_of(me, me ^ rel, LEAD_E - 1) >> (CD.bit_length() - 1)
      for rel in (1, 2, 3)}

  def send_dispatch(lo, hi):
    interleaved(
        [(lo[rel], hi[rel], total(me, me ^ rel),
          lambda c, size, rel=rel: d_own(rel, c, size).start())
         for rel in (2, 3, 1)], DISPATCH)

  send_dispatch({1: 0, 2: 0, 3: 0}, sent_early)
  sort_blocks(LEAD_ROWS, NROW)
  send_dispatch(sent_early,
                {rel: d_sent(rel, jnp.int32(0)) for rel in (1, 2, 3)})

  split = plan_detours()
  split = {rel: _pick(me ^ rel, split) for rel in range(NDEV)}

  def goes_by_y(rel, c):
    return c >= split[rel]

  xe[...] = jnp.zeros(xe.shape, jnp.int32)

  def run_expert(j):
    for rel in (1, 3, 2):
      s = me ^ rel
      each_chunk(d_chunks(s, me, j - 1), d_chunks(s, me, j), total(s, me),
                 DISPATCH, lambda c, size, rel=rel: remote(
                     d_rows(rel, c, size), d_rows(rel, c, size), d_send,
                     d_recv.at[d_in[rel] + c], rel).wait_recv())

    segments, parts = [], []
    filled = jnp.int32(0)
    before = jnp.maximum(j - 1, 0)
    for s in range(NDEV):
      first = jnp.where(j == 0, 0, end_of(s, me, before))
      count = end_of(s, me, j) - first
      segments.append((s ^ me, first, count, filled))
      lead_last = lead_end_of(s, me, j)
      lead = lead_last - jnp.where(j == 0, 0, lead_end_of(s, me, before))
      lead = jnp.where(j < LEAD_E, lead, 0)
      later_leads = jnp.where(
          j < LEAD_E, lead_end_of(s, me, LEAD_E - 1) - lead_last, 0)
      parts.append((s ^ me, lead_last, lead, filled + lead))
      filled = filled + count
      parts.append(
          (s ^ me, first + count + later_leads, count - lead, filled))

    for rel, last, count, to in reversed(parts):
      def copy_in(i, rel=rel, last=last, to=to):
        src = (D_FIRST + rel * LD + last - (i + 1) * DCOPY) * XR
        dst = (DCOPY + to - (i + 1) * DCOPY) * XR
        xe[pl.ds(dst, DCOPY * XR), :] = dbuf[pl.ds(src, DCOPY * XR), :]

      _loop(0, _cdiv_pow2(count, DCOPY), copy_in)

    pieces = []
    for h in range(XR):
      words = xe[pl.ds(DCOPY * XR + h, CP, stride=XR), :]
      pieces += [_unpack(words, 0), _unpack(words, 1)]
    tokens = jnp.concatenate(pieces, axis=1).astype(jnp.bfloat16)
    w_copy(j).wait()
    y_base = pl.multiple_of(j * (CP * YR), CP * YR)
    for c in range(YR):
      w = jnp.concatenate(
          [wbuf[j, :, 128 * k:128 * (k + 1)] for k in (c, c + YR)], axis=1
      ).astype(jnp.bfloat16)
      y = jnp.dot(tokens, w, preferred_element_type=jnp.float32)
      ybuf[pl.ds(y_base + c, CP, stride=YR), :] = _pack(y[:, :128], y[:, 128:])

    for rel, first, count, at in segments:
      slot = jnp.where(rel == 0, 0, rel + 3)

      def copy_out(i, slot=slot, first=first, at=at):
        src = y_base + (at + i * RCOPY) * YR
        dst = (slot * LR + first + i * RCOPY) * YR
        rbuf[pl.ds(dst, RCOPY * YR), :] = ybuf[pl.ds(src, RCOPY * YR), :]

      _loop(0, _cdiv_pow2(count, RCOPY), copy_out)

  def place(home, lo, hi):
    out[pl.ds(home, YR, stride=8), :] = lo
    out[pl.ds(home + 8 * YR, YR, stride=8), :] = hi

  def place_chunk(rel, c, left):
    start = pl.multiple_of((rel * LR + c * CR) * YR, CR * YR)
    per_row = 128 // CR
    row = rel * 16 + (c >> (per_row.bit_length() - 1))
    for part in range(per_row):
      @pl.when((left >= CR) & ((c & (per_row - 1)) == part))
      def _(part=part):
        words = rbuf[pl.ds(start, CR * YR), :]
        lo, hi = _unpack(words, 0), _unpack(words, 1)
        for u in range(CR):
          rows = slice(u * YR, (u + 1) * YR)
          place(home_s[row, part * CR + u], lo[rows], hi[rows])

    @pl.when(left < CR)
    def _():
      def place_one(u):
        words = rbuf[pl.ds(start + u * YR, YR), :]
        home = home_s[row, (c & (per_row - 1)) * CR + u]
        place(home, _unpack(words, 0), _unpack(words, 1))

      _loop(0, left, place_one)

  def own_result(rel, c, size, act):
    if rel != 2:
      act(r_own(rel, c, size))
    else:
      by_y = goes_by_y(0, c)
      pl.when(by_y)(lambda: act(r_diag(1, c, size, 0)))
      pl.when(jnp.logical_not(by_y))(lambda: act(r_diag(3, c, size, 0)))

  def start_return(rel, c, size):
    own_result(rel, c, size, lambda copy: copy.start())

  def passes_here(rel, c):
    by_y = goes_by_y(rel, c)
    return by_y if rel == 1 else jnp.logical_not(by_y)

  def forward_result(rel, c, size):
    @pl.when(passes_here(rel, c))
    def _():
      r_diag(rel, c, size, rel).wait_recv()
      r_fwd(rel, c, size).start()

  def forward_dispatch(j):
    def forward(c, size):
      remote(d_rows(7, c, size), d_rows(7, c, size), d_send, d_pass.at[c],
             3).wait_recv()
      d_fwd(c, size).start()

    each_chunk(d_forwarded(j - 1), d_forwarded(j), total(me ^ 3, me ^ 1),
               DISPATCH, forward)

  def step(j):
    pl.when(j > 0)(lambda: send_dispatch(
        {rel: d_sent(rel, j - 1) for rel in (1, 2, 3)},
        {rel: d_sent(rel, j) for rel in (1, 2, 3)}))
    forward_dispatch(j)

    run_expert(j)

    interleaved(
        [(r_chunks(me ^ rel, me, j - 1), r_chunks(me ^ rel, me, j),
          total(me ^ rel, me),
          lambda c, size, rel=rel: start_return(rel, c, size))
         for rel in (2, 3, 1)], RETURN)

    each_chunk(r_forwarded(j - 1), r_forwarded(j), total(me ^ 1, me ^ 3),
               RETURN, lambda c, size: forward_result(3, c, size))

  _loop(0, NE, step)

  for r in range(NROW):
    row_v[1, r:r + 1, :] = pick_rows(hot[r], my_start.astype(jnp.float32))
  stream_pos = row_v[1].astype(jnp.int32) + rank
  key = jnp.where(kept, owner_rel * 32 + (stream_pos >> 7), -1)
  sub128 = lax.broadcasted_iota(jnp.int32, (128, 128), 0)
  lane128 = lax.broadcasted_iota(jnp.int32, (128, 128), 1).astype(jnp.float32)
  table = jnp.zeros((128, 128), jnp.float32)
  for r in range(NROW):
    digits = jnp.where((sub128 & 16) == 0, lane128, float(r))
    lhs = jnp.where((sub128 & ~16) == key[r:r + 1, :], digits, 0.0)
    rhs = jnp.where((stream_pos[r:r + 1, :] & 127) == sub128, 1.0, 0.0)
    table = table + lax.dot_general(
        lhs.astype(jnp.bfloat16), rhs.astype(jnp.bfloat16),
        (((1,), (1,)), ((), ())), preferred_element_type=jnp.float32,
    )
  table = table.astype(jnp.int32)
  for rel in range(NDEV):
    low = table[32 * rel:32 * rel + 16]
    high = table[32 * rel + 16:32 * rel + 32]
    home_v[16 * rel:16 * (rel + 1), :] = (
        high * 1024 + (low >> 3) * 64 + (low & 7))
  home_cp = pltpu.make_async_copy(home_v, home_s, loc_sem.at[1])
  home_cp.start()

  def clear(i):
    rows = pl.ds(pl.multiple_of(i * 512, 512), 512)
    out[rows, :] = jnp.zeros((512, 128), jnp.float32)

  _loop(0, NT * 8 // 512, clear)
  home_cp.wait()

  last = jnp.int32(NE - 1)
  for rel in (1, 2, 3):
    cnt_copy(rel).wait_send()
    each_chunk(0, d_sent(rel, last), total(me, me ^ rel), DISPATCH,
               lambda c, size, rel=rel: d_own(rel, c, size).wait_send())
  each_chunk(0, d_forwarded(last), total(me ^ 3, me ^ 1), DISPATCH,
             lambda c, size: d_fwd(c, size).wait_send())

  passing = {rel: total(me ^ rel ^ 2, me ^ rel) for rel in (1, 3)}
  coming = [total(me, me ^ rel) for rel in range(NDEV)]

  def receive(rel, c):
    left = _pick(rel, coming) - c * CR

    @pl.when(rel > 0)
    def _():
      _sized(left, RETURN, lambda size: remote(
          r_rows(rel, c, size), r_rows(rel, c, size), r_send,
          r_recv.at[_pick(rel, r_in) + c], 1).wait_recv())

    place_chunk(rel, c, left)

  def comes_last(rel, c):
    return (rel == 2) & goes_by_y(2, c)

  lag = [_per_chip(me, lambda m: LAG[m][rel]) for rel in range(NDEV)]
  first = {1: 0, 3: r_forwarded(last)}

  def forward_round(j):
    for rel in (1, 3):
      s, d = me ^ rel ^ 2, me ^ rel
      each_chunk(jnp.maximum(r_chunks(s, d, j - 1), first[rel]),
                 r_chunks(s, d, j), passing[rel], RETURN,
                 lambda c, size, rel=rel: forward_result(rel, c, size))

    def one(rel):
      due = j - _pick(rel, lag)
      _loop(r_chunks(me, me ^ rel, due - 1), r_chunks(me, me ^ rel, due),
            lambda c: pl.when(jnp.logical_not(comes_last(rel, c)))(
                lambda: receive(rel, c)))

    _loop(0, NDEV, one)

  _loop(0, NE, forward_round)

  def wait_forwards(last_few):
    for rel in (1, 3):
      if rel == 1:
        lo, hi = split[1], _cdiv_pow2(passing[1], CR)
      else:
        lo, hi = 0, split[3]
      most = jnp.maximum(hi - TRAILING, lo)
      each_chunk(most if last_few else lo, hi if last_few else most,
                 passing[rel], RETURN,
                 lambda c, size, rel=rel: r_fwd(rel, c, size).wait_send())

  for rel in (1, 2, 3):
    tokens = total(me ^ rel, me)
    each_chunk(0, _cdiv_pow2(tokens, CR), tokens, RETURN,
               lambda c, size, rel=rel: own_result(
                   rel, c, size, lambda copy: copy.wait_send()))

  todo = []
  for rel in range(NDEV):
    done = r_chunks(me, me ^ rel, last - lag[rel])
    todo.append((done, r_chunks(me, me ^ rel, last)))
  last_diag = jnp.maximum(split[2], todo[2][0])
  by_y = [(0, *todo[0]), (1, *todo[1]), (2, todo[2][0], last_diag)]
  by_x = [(3, *todo[3]), (2, split[2], todo[2][1])]

  def receive_from_back(queue, back):
    rel = c = jnp.int32(-1)
    for part, lo, hi in reversed(queue):
      here = (back >= 0) & (back < hi - lo)
      rel = jnp.where(here, part, rel)
      c = jnp.where(here, hi - 1 - back, c)
      back = back - (hi - lo)
    pl.when(rel >= 0)(lambda: receive(rel, c))

  turns = jnp.maximum(sum(hi - lo for _, lo, hi in by_y),
                      sum(hi - lo for _, lo, hi in by_x))

  def finish(t):
    receive_from_back(by_y, turns - 1 - t)
    receive_from_back(by_x, turns - 1 - t)

  wait_at = jnp.maximum(turns - BEFORE_END, 0)

  def finish_and_wait(t):
    pl.when(t == wait_at)(lambda: wait_forwards(False))
    finish(t)

  _loop(0, jnp.maximum(turns, 1), finish_and_wait)
  wait_forwards(True)


def pallas_dist_moe_cap_ep_tokshard_n2048_d512_e8_h1024_kernel(
    x: jax.Array,
    router_W: jax.Array,
    route_idx: jax.Array,
    expert_W: jax.Array,
):
  del router_W
  i32, f32 = jnp.int32, jnp.float32
  dma = pltpu.SemaphoreType.DMA
  tiles = pl.pallas_call(
      _moe_kernel,
      out_shape=pltpu.VMEM((NT * DH // 128, 128), f32),
      in_specs=[pl.BlockSpec(memory_space=pltpu.HBM)] * 3,
      out_specs=pl.BlockSpec(memory_space=pltpu.VMEM),
      scratch_shapes=[
          pltpu.VMEM((NT, DM), f32),
          pltpu.VMEM((NE, DM, DH), f32),
          pltpu.VMEM((NROW, 128), i32),
          pltpu.VMEM((NT * XR + 8, 128), i32),
          pltpu.VMEM(((D_DUMMY + 8) * XR, 128), i32),
          pltpu.VMEM((9 * LR * YR, 128), i32),
          pltpu.VMEM(((CP + DCOPY) * XR + 8, 128), i32),
          pltpu.VMEM(((NE * CP + RCOPY) * YR, 128), i32),
          pltpu.VMEM((NDEV, 16, 128), i32),
          pltpu.VMEM((2, NROW, 128), f32),
          pltpu.VMEM((NROW, 128), i32),
          pltpu.VMEM((32, 128), i32),
          pltpu.VMEM((NDEV * 16, 128), i32),
          pltpu.SMEM((NROW, 128), i32),
          pltpu.SMEM((32, 128), i32),
          pltpu.SMEM((NDEV * 16, 128), i32),
          dma((NROW,)),
          dma((NE,)),
          dma((3,)),
          dma((NDEV,)),
          dma,
          dma,
          dma,
          dma((MAXS // CD + 3,)),
          dma((NCD,)),
          dma((NT // CR + 3,)),
          dma((NCR + MAX_BY_Y,)),
      ],
      compiler_params=pltpu.CompilerParams(
          vmem_limit_bytes=96 * 1024 * 1024,
          collective_id=0,
          disable_bounds_checks=not CHECKS,
          disable_semaphore_checks=not CHECKS,
      ),
  )(x, route_idx.astype(i32).reshape(NROW, 128), expert_W)
  tiles = tiles.reshape(NT // 8, DH // 128, 8, 128)
  return tiles.transpose(0, 2, 1, 3).reshape(NT, DH)
```
